```python
import numpy as np

kernel_name = "dist_rope_attn_htp_bs_b2_sq512_d1024_hq8_dh128"

def setup_inputs():
    x = np.random.randn(8, 512, 1024).astype(np.float32)
    Wq = np.random.randn(1024, 4096).astype(np.float32) * 0.02
    Wk = np.random.randn(1024, 4096).astype(np.float32) * 0.02
    Wv = np.random.randn(1024, 4096).astype(np.float32) * 0.02
    Wo = np.random.randn(4096, 1024).astype(np.float32) * 0.02
    return {"x": x, "Wq": Wq, "Wk": Wk, "Wv": Wv, "Wo": Wo}

def reference(x, Wq, Wk, Wv, Wo):
    B, Sq, Hq, Dh = 8, 512, 32, 128
    inv = 1.0 / (10000.0 ** (np.arange(0, Dh, 2) / Dh))
    pos = np.arange(Sq)[:, None] * inv[None, :]
    cos = np.repeat(np.cos(pos), 2, axis=-1).astype(np.float32)
    sin = np.repeat(np.sin(pos), 2, axis=-1).astype(np.float32)
    def rot(t):
        t2 = t.reshape(B, Sq, Hq, Dh // 2, 2)
        t_r = np.stack([-t2[..., 1], t2[..., 0]], axis=-1).reshape(B, Sq, Hq, Dh)
        return t * cos[None, :, None, :] + t_r * sin[None, :, None, :]
    Q = rot((x @ Wq).reshape(B, Sq, Hq, Dh))
    K = rot((x @ Wk).reshape(B, Sq, Hq, Dh))
    V = (x @ Wv).reshape(B, Sq, Hq, Dh)
    s = np.einsum('bihd,bjhd->bhij', Q, K).astype(np.float32) * 0.08838834764831843
    s_max = s.max(axis=-1, keepdims=True)
    w = np.exp(s - s_max)
    w = w / w.sum(axis=-1, keepdims=True)
    ctx = np.einsum('bhij,bjhd->bihd', w, V).reshape(B, Sq, Hq * Dh)
    return ctx @ Wo
```

```python
import numpy as np
import jax
import jax.numpy as jnp
from jax import lax
from jax.experimental import pallas as pl
from jax.experimental.pallas import tpu as pltpu

N_DEV = 4
S = 512
D = 1024
DH = 128
HL = 8
CW = 256
NC = D // CW
BF = jnp.bfloat16
F32 = jnp.float32


def _rope_tables():
    inv = 1.0 / (10000.0 ** (np.arange(0, DH, 2) / DH))
    pos = np.arange(S)[:, None] * inv[None, :]
    cos = np.repeat(np.cos(pos), 2, axis=-1)
    sin = np.repeat(np.sin(pos), 2, axis=-1)
    even = (np.arange(DH) % 2 == 0)[None, :]
    sa = np.where(even, -sin, 0.0)
    sb = np.where(even, 0.0, sin)
    c = 0.08838834764831843 * np.log2(np.e)
    return np.stack([cos * c, sa * c, sb * c, cos, sa, sb]).astype(np.float32)


def _body(x_hbm, wq_hbm, wk_hbm, wv_hbm, wo_hbm, tab_ref, out_hbm,
          xf, wst, wb, xg, ctx, ps, rb, acc0, ost,
          xsem, wsem, osem, xs_sem, xr_sem, ps_sem, pr_sem):
    me = lax.axis_index("i")
    left = (me + N_DEV - 1) % N_DEV
    right = (me + 1) % N_DEV

    xcp = [pltpu.make_async_copy(x_hbm.at[b], xf.at[b], xsem.at[b]) for b in range(2)]
    w_hbm = [wq_hbm, wk_hbm, wv_hbm, wo_hbm]

    def wcp(m, c):
        return pltpu.make_async_copy(
            w_hbm[m].at[:, pl.ds(c * CW, CW)], wst.at[m, c], wsem.at[m, c])

    xcp[0].start()
    xcp[1].start()
    for c in range(NC):
        for m in range(3):
            wcp(m, c).start()
    for c in range(NC):
        wcp(3, c).start()

    bar = pltpu.get_barrier_semaphore()
    for nbr in (left, right):
        pl.semaphore_signal(bar, inc=1, device_id=(nbr,),
                            device_id_type=pl.DeviceIdType.MESH)

    def xsend(i, src, dst, dev):
        return pltpu.make_async_remote_copy(
            src_ref=xg.at[src], dst_ref=xg.at[dst],
            send_sem=xs_sem.at[i], recv_sem=xr_sem.at[dst],
            device_id=(dev,), device_id_type=pl.DeviceIdType.MESH)

    def psend(s):
        dev = (left, right, right, left, right, left)[s - 1]
        return pltpu.make_async_remote_copy(
            src_ref=ps.at[s - 1], dst_ref=rb.at[s - 1],
            send_sem=ps_sem.at[s - 1], recv_sem=pr_sem.at[s - 1],
            device_id=(dev,), device_id_type=pl.DeviceIdType.MESH)

    xcp[0].wait()
    xg[0] = xf[0].astype(BF)
    xcp[1].wait()
    xg[7] = xf[1].astype(BF)
    pl.semaphore_wait(bar, 2)
    sends = [xsend(0, 0, 1, right), xsend(1, 7, 2, left),
             xsend(2, 1, 3, right), xsend(3, 2, 4, left),
             xsend(4, 7, 6, right), xsend(5, 0, 5, left)]
    sends[0].start()
    sends[1].start()

    def rope(t, base):
        return (t * tab_ref[base] + pltpu.roll(t, DH - 1, 1) * tab_ref[base + 1]
                + pltpu.roll(t, 1, 1) * tab_ref[base + 2])

    def compute(s, first):
        xb = xg[s]
        for c in range(NC):
            if first:
                for m in range(3):
                    wcp(m, c).wait()
                    wb[m, c] = wst[m, c].astype(BF)
            q2 = jnp.dot(xb, wb[0, c], preferred_element_type=F32)
            k2 = jnp.dot(xb, wb[1, c], preferred_element_type=F32)
            v2 = jnp.dot(xb, wb[2, c], preferred_element_type=F32).astype(BF)
            for j in range(CW // DH):
                sl = slice(j * DH, (j + 1) * DH)
                q = rope(q2[:, sl], 0).astype(BF)
                k = rope(k2[:, sl], 3).astype(BF)
                sc = lax.dot_general(q, k, (((1,), (1,)), ((), ())),
                                     preferred_element_type=F32)
                mx = jnp.max(sc, axis=-1, keepdims=True)
                p = jnp.exp2(sc - mx)
                l = jnp.sum(p, axis=-1, keepdims=True)
                o = jnp.dot(p.astype(BF), v2[:, sl], preferred_element_type=F32)
                h = c * (CW // DH) + j
                ctx[:, h * DH:(h + 1) * DH] = (o * (1.0 / l)).astype(BF)
        if first:
            for c in range(NC):
                wcp(3, c).wait()
                wb[3, c] = wst[3, c].astype(BF)

    def oproj(c):
        return jnp.dot(ctx[...], wb[3, c], preferred_element_type=F32)

    compute(0, True)
    for c in range(NC):
        acc0[:, c * CW:(c + 1) * CW] = oproj(c)

    def step(s, carry):
        for t in range(1, 7):
            @pl.when(s == t)
            def _():
                xsend(0, t, t, left).wait_recv()
                if t == 1:
                    sends[2].start()
                    sends[4].start()
                if t == 2:
                    sends[3].start()
                    sends[5].start()
                if t == 5:
                    psend(3).wait_recv()
                if t == 6:
                    psend(4).wait_recv()
        compute(s, False)

        @pl.when(s < 5)
        def _():
            for c in range(NC):
                ps[s - 1, :, c * CW:(c + 1) * CW] = oproj(c).astype(BF)

        @pl.when(s >= 5)
        def _():
            for c in range(NC):
                cs = slice(c * CW, (c + 1) * CW)
                ps[s - 1, :, cs] = (oproj(c) + rb[s - 3, :, cs].astype(F32)).astype(BF)

        for t in range(1, 7):
            @pl.when(s == t)
            def _():
                psend(t).start()
        return carry

    lax.fori_loop(1, 7, step, 0)

    psend(1).wait_recv()
    psend(5).wait_recv()
    ost[0] = acc0[...] + rb[0].astype(F32) + rb[4].astype(F32)
    ocp0 = pltpu.make_async_copy(ost.at[0], out_hbm.at[0], osem.at[0])
    ocp0.start()

    compute(7, False)
    psend(2).wait_recv()
    psend(6).wait_recv()
    ocps = []
    for c in range(NC):
        cs = slice(c * CW, (c + 1) * CW)
        ost[1, :, cs] = oproj(c) + rb[1, :, cs].astype(F32) + rb[5, :, cs].astype(F32)
        cp = pltpu.make_async_copy(ost.at[1, :, pl.ds(c * CW, CW)],
                                   out_hbm.at[1, :, pl.ds(c * CW, CW)], osem.at[1 + c])
        cp.start()
        ocps.append(cp)
    ocp0.wait()
    for cp in ocps:
        cp.wait()
    for sd in sends:
        sd.wait_send()
    for t in range(1, 7):
        psend(t).wait_send()


def pallas_dist_rope_attn_htp_bs_b2_sq512_d1024_hq8_dh128_kernel(x, Wq, Wk, Wv, Wo):
    tabs = jnp.asarray(_rope_tables())
    any_spec = pl.BlockSpec(memory_space=pl.ANY)
    return pl.pallas_call(
        _body,
        out_shape=jax.ShapeDtypeStruct((2, S, D), F32),
        in_specs=[any_spec] * 5 + [pl.BlockSpec(memory_space=pltpu.VMEM)],
        out_specs=any_spec,
        scratch_shapes=[
            pltpu.VMEM((2, S, D), F32),
            pltpu.VMEM((4, NC, D, CW), F32),
            pltpu.VMEM((4, NC, D, CW), BF),
            pltpu.VMEM((8, S, D), BF),
            pltpu.VMEM((S, D), BF),
            pltpu.VMEM((6, S, D), BF),
            pltpu.VMEM((6, S, D), BF),
            pltpu.VMEM((S, D), F32),
            pltpu.VMEM((2, S, D), F32),
            pltpu.SemaphoreType.DMA((2,)),
            pltpu.SemaphoreType.DMA((4, NC)),
            pltpu.SemaphoreType.DMA((1 + NC,)),
            pltpu.SemaphoreType.DMA((6,)),
            pltpu.SemaphoreType.DMA((8,)),
            pltpu.SemaphoreType.DMA((6,)),
            pltpu.SemaphoreType.DMA((6,)),
        ],
        compiler_params=pltpu.CompilerParams(
            collective_id=0, vmem_limit_bytes=100 * 1024 * 1024),
    )(x, Wq, Wk, Wv, Wo, tabs)
```

```python
import numpy as np
import jax
import jax.numpy as jnp
from jax import lax
from jax.experimental import pallas as pl
from jax.experimental.pallas import tpu as pltpu

N_DEV = 4
S = 512
D = 1024
DH = 128
CW = 256
NC = D // CW
BF = jnp.bfloat16
F32 = jnp.float32


def _fill_rope_tables(tab_ref):
    lane = lax.broadcasted_iota(jnp.int32, (S, DH), 1)
    row = lax.broadcasted_iota(jnp.int32, (S, DH), 0).astype(F32)
    even = (lane & 1) == 0
    pair = (lane - (lane & 1)).astype(F32)
    ang = row * jnp.exp(pair * (-float(np.log(10000.0)) / DH))
    cos = jnp.cos(ang)
    sin = jnp.sin(ang)
    sa = jnp.where(even, -sin, 0.0)
    sb = jnp.where(even, 0.0, sin)
    c = float(0.08838834764831843 * np.log2(np.e))
    for i, t in enumerate((cos * c, sa * c, sb * c, cos, sa, sb)):
        tab_ref[i] = t


def _body(x_hbm, wq_hbm, wk_hbm, wv_hbm, wo_hbm, out_ref,
          tab_ref, xf, wst, xg, ctx, ctx0, ps0, ps, rb,
          xsem, wsem, xs_sem, xr_sem, ps_sem, pr_sem):
    me = lax.axis_index("i")
    left = (me + N_DEV - 1) % N_DEV
    right = (me + 1) % N_DEV

    xcp = [pltpu.make_async_copy(x_hbm.at[b], xf.at[b], xsem.at[b]) for b in range(2)]
    w_hbm = [wq_hbm, wk_hbm, wv_hbm, wo_hbm]

    def wcp(m, c):
        return pltpu.make_async_copy(
            w_hbm[m].at[:, pl.ds(c * CW, CW)], wst.at[m, c], wsem.at[m, c])

    xcp[0].start()
    for m in range(3):
        wcp(m, 0).start()

    bar = pltpu.get_barrier_semaphore()
    for nbr in (left, right):
        pl.semaphore_signal(bar, inc=1, device_id=(nbr,),
                            device_id_type=pl.DeviceIdType.MESH)

    def xsend(i, src, dst, dev):
        return pltpu.make_async_remote_copy(
            src_ref=xg.at[src], dst_ref=xg.at[dst],
            send_sem=xs_sem.at[i], recv_sem=xr_sem.at[dst],
            device_id=(dev,), device_id_type=pl.DeviceIdType.MESH)

    def psend(s):
        dev = (left, right, right, left, right, left)[s - 1]
        return pltpu.make_async_remote_copy(
            src_ref=ps.at[s], dst_ref=rb.at[s - 1],
            send_sem=ps_sem.at[s - 1], recv_sem=pr_sem.at[s - 1],
            device_id=(dev,), device_id_type=pl.DeviceIdType.MESH)

    _fill_rope_tables(tab_ref)
    rb[6] = jnp.zeros((S, D), BF)
    xcp[0].wait()
    xg[0] = xf[0].astype(BF)
    pl.semaphore_wait(bar, 2)
    sends = [xsend(0, 0, 1, right), xsend(1, 7, 2, left),
             xsend(2, 1, 3, right), xsend(3, 2, 4, left),
             xsend(4, 7, 6, right), xsend(5, 0, 5, left)]
    sends[0].start()

    def rope(t, base):
        return (t * tab_ref[base] + pltpu.roll(t, DH - 1, 1) * tab_ref[base + 1]
                + pltpu.roll(t, 1, 1) * tab_ref[base + 2])

    def compute(s, first, c0=None):

        def proj(c):
            q2 = jnp.dot(xg[s], wst[0, c].astype(BF), preferred_element_type=F32)
            k2 = jnp.dot(xg[s], wst[1, c].astype(BF), preferred_element_type=F32)
            v2 = jnp.dot(xg[s], wst[2, c].astype(BF), preferred_element_type=F32).astype(BF)
            r = []
            for j in range(CW // DH):
                sl = slice(j * DH, (j + 1) * DH)
                r.append((rope(q2[:, sl], 0).astype(BF),
                          rope(k2[:, sl], 3).astype(BF), v2[:, sl]))
            return r

        if first:
            for j, (q, k, v) in enumerate(proj(c0)):
                sc = lax.dot_general(q, k, (((1,), (1,)), ((), ())),
                                     preferred_element_type=F32)
                mx = jnp.max(sc, axis=-1, keepdims=True)
                p = jnp.exp2(sc - mx)
                l = jnp.sum(p, axis=-1, keepdims=True)
                o = jnp.dot(p.astype(BF), v, preferred_element_type=F32)
                ctx0[c0, :, j * DH:(j + 1) * DH] = (o * (1.0 / l)).astype(BF)
            return
        nxt = proj(0)
        for c in range(NC):
            cur = nxt
            scs = [lax.dot_general(q, k, (((1,), (1,)), ((), ())),
                                   preferred_element_type=F32) for q, k, _ in cur]
            if c + 1 < NC:
                nxt = proj(c + 1)
            for j, sc in enumerate(scs):
                mx = jnp.max(sc, axis=-1, keepdims=True)
                p = jnp.exp2(sc - mx)
                l = jnp.sum(p, axis=-1, keepdims=True)
                o = jnp.dot(p.astype(BF), cur[j][2], preferred_element_type=F32)
                h = c * (CW // DH) + j
                ctx[:, h * DH:(h + 1) * DH] = (o * (1.0 / l)).astype(BF)

    def oproj(c):
        return jnp.dot(ctx[...], wst[3, c].astype(BF), preferred_element_type=F32)

    def chunk0(c, carry):
        for m in range(3):
            wcp(m, c).wait()

        @pl.when(c + 1 < NC)
        def _():
            for m in range(3):
                wcp(m, c + 1).start()

        @pl.when(c + 1 == NC)
        def _():
            for cc in range(NC):
                wcp(3, cc).start()

        compute(0, True, c)
        return carry

    lax.fori_loop(0, NC, chunk0, 0)

    def oproj0(c, carry):
        wcp(3, c).wait()

        @pl.when(c == 1)
        def _():
            xcp[1].start()

        lhs = jnp.concatenate([ctx0[i] for i in range(NC)], axis=1)
        ps0[c] = jnp.dot(lhs, wst[3, c].astype(BF),
                         preferred_element_type=F32).astype(BF)
        return carry

    lax.fori_loop(0, NC, oproj0, 0)

    xcp[1].wait()
    xg[7] = xf[1].astype(BF)
    sends[1].start()

    def step(s, carry):
        for t in range(1, 7):
            @pl.when(s == t)
            def _():
                xsend(0, t, t, left).wait_recv()
                if t == 1:
                    sends[2].start()
                    sends[4].start()
                if t == 2:
                    sends[3].start()
                    sends[5].start()
                if t == 5:
                    psend(3).wait_recv()
                if t == 6:
                    psend(4).wait_recv()
        @pl.when(s == 7)
        def _():
            psend(1).wait_recv()
            psend(5).wait_recv()
            for c in range(NC):
                cs = slice(c * CW, (c + 1) * CW)
                out_ref[0, :, cs] = (ps0[c].astype(F32) + rb[0, :, cs].astype(F32)
                                     + rb[4, :, cs].astype(F32)).astype(BF)

        compute(s, False)

        ai = jnp.where((s == 5) | (s == 6), s - 3, 6)
        for c in range(NC):
            cs = slice(c * CW, (c + 1) * CW)
            ps[s, :, cs] = (oproj(c) + rb[ai, :, cs].astype(F32)).astype(BF)

        for t in range(1, 7):
            @pl.when(s == t)
            def _():
                psend(t).start()
        return carry

    lax.fori_loop(1, 8, step, 0)
    psend(2).wait_recv()
    psend(6).wait_recv()
    out_ref[1] = (ps[7].astype(F32) + rb[1].astype(F32) + rb[5].astype(F32)).astype(BF)
    for sd in sends:
        sd.wait_send()
    for t in range(1, 7):
        psend(t).wait_send()


def pallas_dist_rope_attn_htp_bs_b2_sq512_d1024_hq8_dh128_kernel(x, Wq, Wk, Wv, Wo):
    any_spec = pl.BlockSpec(memory_space=pltpu.MemorySpace.HBM)
    return pl.pallas_call(
        _body,
        out_shape=jax.ShapeDtypeStruct((2, S, D), BF),
        in_specs=[any_spec] * 5,
        out_specs=pl.BlockSpec(memory_space=pltpu.VMEM),
        scratch_shapes=[
            pltpu.VMEM((6, S, DH), F32),
            pltpu.VMEM((2, S, D), F32),
            pltpu.VMEM((4, NC, D, CW), F32),
            pltpu.VMEM((8, S, D), BF),
            pltpu.VMEM((S, D), BF),
            pltpu.VMEM((NC, S, CW), BF),
            pltpu.VMEM((NC, S, CW), BF),
            pltpu.VMEM((8, S, D), BF),
            pltpu.VMEM((7, S, D), BF),
            pltpu.SemaphoreType.DMA((2,)),
            pltpu.SemaphoreType.DMA((4, NC)),
            pltpu.SemaphoreType.DMA((6,)),
            pltpu.SemaphoreType.DMA((8,)),
            pltpu.SemaphoreType.DMA((6,)),
            pltpu.SemaphoreType.DMA((6,)),
        ],
        compiler_params=pltpu.CompilerParams(
            collective_id=0, vmem_limit_bytes=100 * 1024 * 1024),
    )(x, Wq, Wk, Wv, Wo)
```
